```python
import numpy as np

kernel_name = "dist_sparse_attn_strided_kvseq_b1_sq256_skv4096_hq8_dh128"

def setup_inputs():
    x = np.random.randn(1, 256, 1024).astype(np.float32)
    Wq = np.random.randn(1024, 1024).astype(np.float32) * 0.02
    K_ext = np.random.randn(1, 16384, 8, 128).astype(np.float32)
    V_ext = np.random.randn(1, 16384, 8, 128).astype(np.float32)
    Wo = np.random.randn(1024, 1024).astype(np.float32) * 0.02
    return {"x": x, "Wq": Wq, "K_ext": K_ext, "V_ext": V_ext, "Wo": Wo}

def reference(x, Wq, K_ext, V_ext, Wo):
    B, Sq, Skv, Hq, Dh = 1, 256, 16384, 8, 128
    Q = (x @ Wq).reshape(B, Sq, Hq, Dh)
    qb = (np.arange(Sq) // 64)[:, None]
    kb = (np.arange(Skv) // 64)[None, :]
    mask = (qb == kb) | ((kb % 4) == (qb % 4))
    scores = np.einsum('bihd,bjhd->bhij', Q, K_ext).astype(np.float32) * 0.08838834764831843
    scores = np.where(mask[None, None, :, :], scores, -1e9)
    scores_max = scores.max(axis=-1, keepdims=True)
    w = np.exp(scores - scores_max)
    row_keep = mask.any(axis=1)
    w_sum = np.where(row_keep[None, None, :, None], w.sum(axis=-1, keepdims=True), 1.0)
    w = w / w_sum
    w = np.where(row_keep[None, None, :, None], w, 0.0)
    ctx = np.einsum('bhij,bjhd->bihd', w, V_ext).reshape(B, Sq, Hq * Dh)
    return ctx @ Wo
```

```python
import contextlib
import jax
import jax.numpy as jnp
from jax import lax
from jax.experimental import pallas as pl
from jax.experimental.pallas import tpu as pltpu

NDEV, NH, QB, DH, NBLK, DM = 4, 8, 64, 128, 16, 1024
NKEY = NBLK * QB
NUNIT = NDEV * NH
QSCALE = 0.08838834764831843 * 1.4426950408889634
F32, BF16 = jnp.float32, jnp.bfloat16
MESH = pl.DeviceIdType.MESH


def build(share_x=True, early=(7, 0, 1), first=10, second=17, ahead=11, out_dtype=BF16, prof=False,
          sem_checks=False, bounds=False):
    late = tuple(h for h in range(NH) if h not in early)
    scope = jax.named_scope if prof else (lambda name: contextlib.nullcontext())

    def body(x_hbm, wq_hbm, k_hbm, v_hbm, wo_hbm, out_ref,
             x_f32, wq_f32, wo_f32, x_all, q_all, wo_all, kbuf, vbuf, part_out, part_in, ctx, acc,
             w_sem, wo_sem, k_sem, v_sem, send_sem, x_rsem, q_rsem, wo_rsem, part_rsem, ctx_rsem, last_rsem):
        me = lax.axis_index("i")

        def peer(d):
            return ((me + d) % NDEV,)

        def k_copy(u):
            c = (me + 1 + u // NH) % NDEV
            return pltpu.make_async_copy(k_hbm.at[:, c, :, u % NH], kbuf.at[u], k_sem.at[u])

        def v_copy(u):
            c = (me + 1 + u // NH) % NDEV
            return pltpu.make_async_copy(v_hbm.at[:, c, :, u % NH], vbuf.at[u], v_sem.at[u])

        def wo_late_copy(h):
            rows = pl.ds(h * DH, DH)
            return pltpu.make_async_copy(wo_hbm.at[rows], wo_f32.at[rows], wo_sem.at[h])

        def fetch(u):
            k_copy(u).start()
            v_copy(u).start()

        my_rows = pl.ds(pl.multiple_of(me * QB, QB), QB)
        if share_x:
            x_copy = pltpu.make_async_copy(x_hbm.at[my_rows], x_f32, w_sem.at[0])
        else:
            x_copy = pltpu.make_async_copy(x_hbm, x_f32, w_sem.at[0])
        wq_copy = pltpu.make_async_copy(
            wq_hbm.at[:, pl.ds(pl.multiple_of(me * 2 * DH, 2 * DH), 2 * DH)], wq_f32, w_sem.at[1])
        x_copy.start()
        wq_copy.start()
        if early:
            shares_wo = me != 2
            my_head = jnp.where(me == 0, early[0], jnp.where(me == 1, early[1], early[2]))
            wo_rows = pl.ds(pl.multiple_of(my_head * DH, DH), DH)
            wo_copy = pltpu.make_async_copy(wo_hbm.at[wo_rows], wo_f32.at[wo_rows], w_sem.at[2])

            @pl.when(shares_wo)
            def _():
                wo_copy.start()

        lax.fori_loop(0, first, lambda u, _: fetch(u), None)

        barrier = pltpu.get_barrier_semaphore()
        for d in (2, 1, 3):
            pl.semaphore_signal(barrier, inc=1, device_id=peer(d), device_id_type=MESH)

        with scope("x"):
            x_copy.wait()
            if share_x:
                x_all[my_rows, :] = x_f32[...].astype(BF16)
            else:
                x_all[...] = x_f32[...].astype(BF16)
        with scope("barrier"):
            pl.semaphore_wait(barrier, NDEV - 1)
        if share_x:
            with scope("x_ag"):
                for d in (1, 3, 2):
                    pltpu.make_async_remote_copy(x_all.at[my_rows], x_all.at[my_rows], send_sem.at[0], x_rsem,
                                                 device_id=peer(d), device_id_type=MESH).start()
                three = x_all.at[pl.ds(0, 3 * QB)]
                pltpu.make_async_copy(three, three, x_rsem).wait()
        lax.fori_loop(first, second, lambda u, _: fetch(u), None)
        with scope("q"):
            wq_copy.wait()
            q = jnp.dot(x_all[...], wq_f32[...].astype(BF16), preferred_element_type=F32) * QSCALE
            q_all[2 * me] = q[:, :DH].astype(BF16)
            q_all[2 * me + 1] = q[:, DH:].astype(BF16)
            mine = q_all.at[pl.ds(2 * me, 2)]
            for d in (1, 3, 2):
                pltpu.make_async_remote_copy(mine, mine, send_sem.at[1], q_rsem,
                                             device_id=peer(d), device_id_type=MESH).start()
        if early:
            with scope("wo_share"):
                @pl.when(shares_wo)
                def _():
                    wo_copy.wait()
                    wo_all[wo_rows, :] = wo_f32[wo_rows, :].astype(BF16)
                    for d in (1, 3, 2):
                        pltpu.make_async_remote_copy(wo_all.at[wo_rows], wo_all.at[wo_rows], send_sem.at[2], wo_rsem,
                                                     device_id=peer(d), device_id_type=MESH).start()
        with scope("q_ag"):
            six = q_all.at[pl.ds(0, 6)]
            pltpu.make_async_copy(six, six, q_rsem).wait()

        lane = lax.broadcasted_iota(jnp.int32, (8, DH), 1)

        def scores(u, c):
            k_copy(u).wait()
            qc = q_all[u % NH, pl.ds(pl.multiple_of(c * QB, QB), QB), :]
            k = kbuf[u].reshape(NKEY, DH).astype(BF16)
            return lax.dot_general(qc, k, (((1,), (1,)), ((), ())), preferred_element_type=F32)

        def weighted(u, p):
            v_copy(u).wait()
            return jnp.dot(p, vbuf[u].reshape(NKEY, DH).astype(BF16), preferred_element_type=F32)

        def other_unit(u, _):
            @pl.when(jnp.logical_and(u + ahead >= second, u + ahead < NUNIT))
            def _():
                fetch(u + ahead)

            phase = u // NH
            c = (me + 1 + phase) % NDEV
            s = scores(u, c)
            m = jnp.max(s, axis=1, keepdims=True)
            p = jnp.exp2(s - m)
            l = jnp.sum(p, axis=1, keepdims=True)
            stats = jnp.zeros((8, DH), F32)
            for g in range(8):
                stats = jnp.where(lane == g, m[8 * g:8 * g + 8], stats)
                stats = jnp.where(lane == 8 + g, l[8 * g:8 * g + 8], stats)
            part_out[u, pl.ds(QB, 16), :] = pltpu.bitcast(stats, BF16)
            part_out[u, pl.ds(0, QB), :] = weighted(u, p.astype(BF16)).astype(BF16)
            pltpu.make_async_remote_copy(part_out.at[u], part_in.at[u % NH, phase], send_sem.at[3],
                                         part_rsem.at[u % NH], device_id=(c,), device_id_type=MESH).start()

        with scope("others"):
            lax.fori_loop(0, NUNIT - NH, other_unit, None)

        for h in late:
            wo_late_copy(h).start()

        def spread(stats, first_lane):
            return jnp.concatenate(
                [jnp.broadcast_to(stats[:, first_lane + g:first_lane + g + 1], (8, DH)) for g in range(8)], axis=0)

        def own_unit(h, last):
            u = NUNIT - NH + h
            s = scores(u, me)
            pltpu.make_async_copy(part_in.at[h], part_in.at[h], part_rsem.at[h]).wait()
            stats = [pltpu.bitcast(part_in[h, j, pl.ds(QB, 16), :], F32) for j in range(3)]
            ms = [spread(st, 0) for st in stats]
            m = jnp.max(s, axis=1, keepdims=True)
            m = jnp.maximum(jnp.maximum(ms[0], ms[1]), jnp.maximum(ms[2], m))
            p = jnp.exp2(s - jnp.tile(m, (1, NKEY // DH)))
            l = jnp.sum(p, axis=1, keepdims=True)
            o = None
            for j in range(3):
                a = jnp.exp2(ms[j] - m)
                l = l + a * spread(stats[j], 8)
                t = a * part_in[h, j, pl.ds(0, QB), :].astype(F32)
                o = t if o is None else o + t
            inv = 1.0 / l
            ctx[h, my_rows, :] = ((o + weighted(u, p.astype(BF16))) * inv).astype(BF16)
            for d in (2, 1, 3):
                pltpu.make_async_remote_copy(ctx.at[h, my_rows], ctx.at[h, my_rows], send_sem.at[4],
                                             last_rsem.at[d - 1] if last else ctx_rsem.at[h],
                                             device_id=peer(d), device_id_type=MESH).start()

        def ctx_wait(h):
            three = ctx.at[h, pl.ds(0, 3 * QB)]
            pltpu.make_async_copy(three, three, ctx_rsem.at[h]).wait()

        with scope("own"):
            lax.fori_loop(0, NH - 1, lambda h, _: own_unit(h, False), None)

        pre = [h for h in early if h != NH - 1]
        if early:
            with scope("wo_wait"):
                @pl.when(shares_wo)
                def _():
                    two = wo_all.at[pl.ds(0, 2 * DH)]
                    pltpu.make_async_copy(two, two, wo_rsem).wait()

                @pl.when(jnp.logical_not(shares_wo))
                def _():
                    three = wo_all.at[pl.ds(0, 3 * DH)]
                    pltpu.make_async_copy(three, three, wo_rsem).wait()
        with scope("proj_early"):
            t = None
            for h in pre:
                ctx_wait(h)
            for h in pre:
                d = jnp.dot(ctx[h], wo_all[pl.ds(h * DH, DH), :], preferred_element_type=F32)
                t = d if t is None else t + d
            acc[...] = jnp.zeros(acc.shape, F32) if t is None else t
        with scope("last_unit"):
            own_unit(NH - 1, True)

        def proj_late(i, _):
            h = late[0] + i
            ctx_wait(h)
            wo_late_copy(h).wait()
            w = wo_f32[pl.ds(pl.multiple_of(h * DH, DH), DH), :].astype(BF16)
            acc[...] += jnp.dot(ctx[h], w, preferred_element_type=F32)

        with scope("proj_late"):
            lax.fori_loop(0, len([h for h in late if h != NH - 1]), proj_late, None)
        if NH - 1 in late:
            wo_late_copy(NH - 1).wait()
            wo_all[pl.ds((NH - 1) * DH, DH), :] = wo_f32[pl.ds((NH - 1) * DH, DH), :].astype(BF16)

        for d in (0, 1, 3, 2):
            with scope(f"final{d}"):
                src = (me + NDEV - d) % NDEV
                rows = pl.ds(pl.multiple_of(src * QB, QB), QB)
                if d:
                    blk = ctx.at[NH - 1, rows]
                    pltpu.make_async_copy(blk, blk, last_rsem.at[d - 1]).wait()
                o = jnp.dot(ctx[NH - 1, rows, :], wo_all[pl.ds((NH - 1) * DH, DH), :], preferred_element_type=F32)
                out_ref[rows, :] = (acc[rows, :] + o).astype(out_ref.dtype)

        with scope("drain"):
            def drain(ref, sem):
                pltpu.make_async_copy(ref, ref, sem).wait()

            if share_x:
                drain(x_all.at[pl.ds(0, 3 * QB)], send_sem.at[0])
            drain(q_all.at[pl.ds(0, 6)], send_sem.at[1])
            if early:
                @pl.when(shares_wo)
                def _():
                    drain(wo_all.at[pl.ds(0, 3 * DH)], send_sem.at[2])
            drain(part_out, send_sem.at[3])
            drain(ctx.at[pl.ds(0, 6)], send_sem.at[4])

    def fn(x, Wq, K_ext, V_ext, Wo):
        dma = pltpu.SemaphoreType.DMA
        out = pl.pallas_call(
            body,
            out_shape=jax.ShapeDtypeStruct((NDEV * QB, DM), out_dtype),
            in_specs=[pl.BlockSpec(memory_space=pl.ANY)] * 5,
            out_specs=pl.BlockSpec(memory_space=pltpu.VMEM),
            scratch_shapes=[
                pltpu.VMEM((QB if share_x else NDEV * QB, DM), F32),
                pltpu.VMEM((DM, 2 * DH), F32),
                pltpu.VMEM((DM, DM), F32),
                pltpu.VMEM((NDEV * QB, DM), BF16),
                pltpu.VMEM((NH, NDEV * QB, DH), BF16),
                pltpu.VMEM((DM, DM), BF16),
                pltpu.VMEM((NUNIT, NBLK, QB, DH), F32),
                pltpu.VMEM((NUNIT, NBLK, QB, DH), F32),
                pltpu.VMEM((NUNIT - NH, QB + 16, DH), BF16),
                pltpu.VMEM((NH, 3, QB + 16, DH), BF16),
                pltpu.VMEM((NH, NDEV * QB, DH), BF16),
                pltpu.VMEM((NDEV * QB, DM), F32),
                dma((3,)), dma((NH,)), dma((NUNIT,)), dma((NUNIT,)), dma((5,)),
                dma, dma, dma, dma((NH,)), dma((NH,)), dma((3,)),
            ],
            compiler_params=pltpu.CompilerParams(
                vmem_limit_bytes=64 * 2**20, collective_id=0,
                disable_semaphore_checks=not sem_checks, disable_bounds_checks=not bounds),
        )(x.reshape(NDEV * QB, DM), Wq, K_ext.reshape(NBLK, NDEV, QB, NH, DH),
          V_ext.reshape(NBLK, NDEV, QB, NH, DH), Wo)
        return out.reshape(1, NDEV * QB, DM)

    return fn


pallas_dist_sparse_attn_strided_kvseq_b1_sq256_skv4096_hq8_dh128_kernel = build()
```

```python
import jax
import jax.numpy as jnp
from jax import lax
from jax.experimental import pallas as pl
from jax.experimental.pallas import tpu as pltpu

NDEV = 4
HEADS, DH = 8, 128
DMODEL = HEADS * DH
QBLK = 64
SQ = NDEV * QBLK
KBLKS = 16
KEYS = KBLKS * QBLK
UNITS = NDEV * HEADS
COMMON = UNITS - 1
LAST_HEAD = HEADS - 1
KSPLIT = DMODEL // NDEV
HALF = DMODEL // 2
PACKED = QBLK // 2

QSCALE = 0.08838834764831843 * 1.4426950408889634

WO_PIECE = {1: (0, 144), 3: (144, 192), 0: (336, 176)}
RELAY = 2
SHARED_HEADS = 4
WO_CUTS = (0, 64, 96)

PREFETCH = (9, 11, 18, 24)
LOOKAHEAD = 11
RELAY_UNIT = 5
PROJECT_LAG = 3

F32, BF16, U32 = jnp.float32, jnp.bfloat16, jnp.uint32


def _block(index, size):
    start = index * size
    return pl.ds(start if isinstance(index, int) else pl.multiple_of(start, size), size)


def _wo_chunk(chip, t):
    first, rows = WO_PIECE[chip]
    end = WO_CUTS[t + 1] if t + 1 < len(WO_CUTS) else rows
    return pl.ds(first + WO_CUTS[t], end - WO_CUTS[t])


def _wait_filled(ref, sem):
    pltpu.make_async_copy(ref, ref, sem).wait()


def _remote(src, dst, send_sem, recv_sem, target):
    return pltpu.make_async_remote_copy(
        src, dst, send_sem, recv_sem,
        device_id=(target,), device_id_type=pl.DeviceIdType.MESH)


def _dot(a, b):
    return jnp.dot(a, b, preferred_element_type=F32)


def _pack_stats(m, l):
    lane = lax.broadcasted_iota(jnp.int32, (8, DH), 1)
    stats = jnp.zeros((8, DH), F32)
    for g in range(8):
        stats = jnp.where(lane == g, m[8 * g:8 * g + 8], stats)
        stats = jnp.where(lane == 8 + g, l[8 * g:8 * g + 8], stats)
    return stats


def _merge_stats(tiles):
    maxima = [t[:, :8] for t in tiles]
    top = maxima[0]
    for m in maxima[1:]:
        top = jnp.maximum(top, m)
    factors = [jnp.exp2(m - top) for m in maxima]
    total = sum(f * t[:, 8:16] for f, t in zip(factors, tiles))
    return top, factors, total


def _spread(packed):
    return jnp.concatenate(
        [jnp.broadcast_to(packed[:, g:g + 1], (8, DH)) for g in range(8)], axis=0)


def _kernel(
    x_hbm, wq_hbm, k_hbm, v_hbm, wo_hbm, out_ref,
    x_buf, wq_buf, wo_buf, k_buf, v_buf,
    qpart, qpart_out, qpart_in, q_all, wo_all, probs, stats,
    part_out, part_in, ctx, common, acc,
    w_sem, wo_sem, k_sem, v_sem,
    qpart_send, qpart_recv, q_send, q_recv, wo_send, wo_recv,
    part_send, part_recv, ctx_send, ctx_recv,
    stats_send, stats_recv, common_send, common_recv,
):
    me = lax.axis_index("i")

    def peer(d):
        return (me + d) & (NDEV - 1)

    def on(chip, fn):
        pl.when(me == chip)(fn)

    n_foreign = jnp.where(me == 0, UNITS - HEADS, UNITS - HEADS - 1)

    def class_and_head(u):
        if isinstance(u, int):
            return 0, LAST_HEAD
        h = lax.div(u, NDEV - 1)
        c = NDEV - 1 - (u - (NDEV - 1) * h)
        c = jnp.where(c <= me, c - 1, c)
        foreign = u < n_foreign
        return jnp.where(foreign, c, me), jnp.where(foreign, h, u - n_foreign)

    def k_copy(u):
        c, h = class_and_head(u)
        return pltpu.make_async_copy(k_hbm.at[:, c, :, h], k_buf.at[u], k_sem.at[u])

    def v_copy(u):
        c, h = class_and_head(u)
        return pltpu.make_async_copy(v_hbm.at[:, c, :, h], v_buf.at[u], v_sem.at[u])

    def v_common_copy(j):
        blocks = _block(j, KBLKS // 2)
        return pltpu.make_async_copy(
            v_hbm.at[blocks, 0, :, LAST_HEAD], v_buf.at[COMMON, blocks], v_sem.at[COMMON + j])

    def wo_copy(rows, sem, cols=pl.ds(0, DMODEL)):
        return pltpu.make_async_copy(wo_hbm.at[rows, cols], wo_buf.at[rows, cols], sem)

    def wo_head_copy(h):
        return wo_copy(_block(h, DH), wo_sem.at[h])

    def wo_last_copy(j):
        return wo_copy(_block(LAST_HEAD, DH), wo_sem.at[LAST_HEAD + j], _block(j, HALF))

    def wo_cast(rows, sem):
        wo_copy(rows, sem).wait()
        wo_all[rows, :] = wo_buf[rows, :].astype(BF16)

    def wo_rest(chip):
        first, rows = WO_PIECE[chip]
        return pl.ds(first + WO_CUTS[1], rows - WO_CUTS[1])

    def fetch(u, _=None):
        k_copy(u).start()
        v_copy(u).start()

    def qpart_copy(d):
        return _remote(qpart_out.at[peer(d)], qpart_in.at[d - 1],
                       qpart_send.at[d - 1], qpart_recv, peer(d))

    def q_copy(d, owner):
        heads = q_all.at[pl.ds(2 * owner, 2)]
        return _remote(heads, heads, q_send.at[d - 1], q_recv.at[d - 1], peer(d))

    def wo_share_copy(chip, t, side, target):
        rows = wo_all.at[_wo_chunk(chip, t)]
        return _remote(rows, rows, wo_send.at[2 * t + side], wo_recv.at[NDEV * t + chip], target)

    def wo_outgoing(sender, t):
        if sender == RELAY:
            return [wo_share_copy(1, t, 0, 3), wo_share_copy(3, t, 1, 1)]
        return [wo_share_copy(sender, t, side, (sender + d) % NDEV)
                for side, d in enumerate((1, 3))]

    def wo_forward(sender, t):
        if sender == RELAY:
            for copy in wo_outgoing(sender, t):
                copy.wait_recv()
        for copy in wo_outgoing(sender, t):
            copy.start()

    def part_copy(u):
        c, h = class_and_head(u)
        return _remote(part_out.at[u], part_in.at[h, jnp.where(me > c, me - 1, me)],
                       part_send.at[u], part_recv.at[h], c)

    def ctx_copy(h, d, owner):
        rows = ctx.at[h, _block(owner, QBLK)]
        slot = (NDEV - 1) * h + d - 1
        return _remote(rows, rows, ctx_send.at[slot], ctx_recv.at[slot], peer(d))

    def stats_copy(d):
        return _remote(stats.at[0], stats.at[d], stats_send.at[d - 1], stats_recv, peer(d))

    def common_copy(d):
        return _remote(common.at[0], common.at[d], common_send.at[d - 1], common_recv, peer(d))

    def load_projection(j, _):
        rows = _block(j, SQ // 2)
        pltpu.make_async_copy(
            x_hbm.at[rows, _block(me, KSPLIT)], x_buf.at[rows], w_sem.at[0]).start()
        pltpu.make_async_copy(
            wq_hbm.at[_block(2 * me + j, KSPLIT // 2)], wq_buf.at[_block(j, KSPLIT // 2)],
            w_sem.at[1]).start()

    for chip in WO_PIECE:
        on(chip, lambda chip=chip: wo_copy(_wo_chunk(chip, 0), w_sem.at[2]).start())
    lax.fori_loop(0, 2, load_projection, None)
    for chip in WO_PIECE:
        on(chip, lambda chip=chip: wo_copy(wo_rest(chip), w_sem.at[3]).start())

    barrier = pltpu.get_barrier_semaphore()
    for d in (2, 1, 3):
        pl.semaphore_signal(barrier, inc=1, device_id=(peer(d),),
                            device_id_type=pl.DeviceIdType.MESH)
    lax.fori_loop(0, PREFETCH[0], fetch, None)
    acc[...] = jnp.zeros(acc.shape, F32)

    for chip in WO_PIECE:
        on(chip, lambda chip=chip: wo_cast(_wo_chunk(chip, 0), w_sem.at[2]))
    pl.semaphore_wait(barrier, NDEV - 1)
    for chip in WO_PIECE:
        on(chip, lambda chip=chip: wo_forward(chip, 0))

    _wait_filled(x_buf, w_sem.at[0])
    _wait_filled(wq_buf, w_sem.at[1])
    q = _dot(x_buf[...].astype(BF16), wq_buf[...].astype(BF16)) * QSCALE
    for j in range(NDEV):
        q_cols = q[:, 2 * DH * j:2 * DH * (j + 1)]
        qpart[j] = q_cols
        qpart_out[j] = q_cols.astype(BF16)
    for d in (1, 3, 2):
        qpart_copy(d).start()

    for chip in WO_PIECE:
        on(chip, lambda chip=chip: wo_cast(wo_rest(chip), w_sem.at[3]))
    for chip in WO_PIECE:
        on(chip, lambda chip=chip: wo_forward(chip, 1))
    lax.fori_loop(PREFETCH[0], PREFETCH[1], fetch, None)
    on(RELAY, lambda: wo_forward(RELAY, 0))

    _wait_filled(qpart_in, qpart_recv)
    lax.fori_loop(PREFETCH[1], PREFETCH[2], fetch, None)
    q = qpart[me] + sum(qpart_in[j].astype(F32) for j in range(NDEV - 1))
    q_all[2 * me] = q[:, :DH].astype(BF16)
    q_all[2 * me + 1] = q[:, DH:].astype(BF16)
    for d in (1, 3, 2):
        q_copy(d, me).start()

    for chip in WO_PIECE:
        on(chip, lambda chip=chip: wo_forward(chip, 2))
    on(RELAY, lambda: wo_forward(RELAY, 1))

    for d in (1, 3, 2):
        q_copy(d, peer(NDEV - d)).wait_recv()
    lax.fori_loop(PREFETCH[2], PREFETCH[3], fetch, None)

    def scores(u):
        c, h = class_and_head(u)
        k = k_buf[u].reshape(KEYS, DH).astype(BF16)
        return lax.dot_general(q_all[h, _block(c, QBLK), :], k, (((1,), (1,)), ((), ())),
                               preferred_element_type=F32)

    def values(u):
        return v_buf[u].reshape(KEYS, DH).astype(BF16)

    def local_softmax(u):
        s = scores(u)
        m = jnp.max(s, axis=1, keepdims=True)
        p = jnp.exp2(s - m)
        stats[0] = _pack_stats(m, jnp.sum(p, axis=1, keepdims=True))
        probs[0] = p[:, :KEYS // 2].astype(BF16)
        probs[1] = p[:, KEYS // 2:].astype(BF16)

    def store_partial(u):
        o = _dot(jnp.concatenate([probs[0], probs[1]], axis=1), values(u))
        part_out[u, pl.ds(PACKED, 8), :] = pltpu.bitcast(stats[0], U32)
        part_out[u, pl.ds(0, PACKED), :] = pltpu.bitcast(o.astype(BF16), U32)

    def foreign_step(u, _):
        ahead = u + LOOKAHEAD
        pl.when(jnp.logical_and(ahead >= PREFETCH[3], ahead < COMMON))(lambda: fetch(ahead))
        pl.when(jnp.logical_and(u == RELAY_UNIT, me == RELAY))(lambda: wo_forward(RELAY, 2))
        v_copy(u).wait()
        k_copy(u + 1).wait()
        store_partial(u)
        local_softmax(u + 1)
        part_copy(u).start()

    k_copy(jnp.int32(0)).wait()
    local_softmax(jnp.int32(0))
    lax.fori_loop(0, n_foreign - 1, foreign_step, None)
    v_copy(n_foreign - 1).wait()
    store_partial(n_foreign - 1)
    part_copy(n_foreign - 1).start()

    first = jnp.where(me == 0, 1, NDEV - me)
    second = jnp.where(first == 2, 1, NDEV - first)
    send_order = (first, second, 6 - first - second)

    def ctx_wait(h):
        for d in range(1, NDEV):
            ctx_copy(h, d, peer(NDEV - d)).wait_recv()

    def project_shared(h, _=None):
        ctx_wait(h)
        acc[...] += _dot(ctx[h], wo_all[_block(h, DH), :])

    def wo_arrivals(chip):
        for t in range(len(WO_CUTS)):
            for source in WO_PIECE:
                if source != chip:
                    wo_share_copy(source, t, 0, source).wait_recv()

    def wo_wait():
        for chip in WO_PIECE:
            on(chip, lambda chip=chip: wo_arrivals(chip))

    relay_rows = pl.ds(*WO_PIECE[0])
    late_reads = (
        lambda: k_copy(COMMON).start(),
        lambda: v_common_copy(0).start(),
        lambda: v_common_copy(1).start(),
        lambda: on(RELAY, lambda: wo_copy(relay_rows, w_sem.at[3]).start()),
        lambda: lax.fori_loop(SHARED_HEADS, LAST_HEAD, lambda h, _: wo_head_copy(h).start(), None),
        lambda: wo_last_copy(0).start(),
        lambda: wo_last_copy(1).start(),
    )
    projected = jnp.where(me == RELAY, WO_PIECE[0][0] // DH, SHARED_HEADS - 1)

    def own_step(h, _):
        for step, start in enumerate(late_reads):
            pl.when(h == step)(start)
        u = n_foreign + h
        _wait_filled(part_in.at[h], part_recv.at[h])
        m_in, factors, l_in = _merge_stats(
            [pltpu.bitcast(part_in[h, j, pl.ds(PACKED, 8), :], F32) for j in range(NDEV - 1)])
        m_in, l_in = _spread(m_in), _spread(l_in)
        o_in = sum(
            _spread(f) * pltpu.bitcast(part_in[h, j, pl.ds(0, PACKED), :], BF16).astype(F32)
            for j, f in enumerate(factors))
        k_copy(u).wait()
        s = scores(u)
        m = jnp.maximum(m_in, jnp.max(s, axis=1, keepdims=True))
        p = jnp.exp2(s - jnp.concatenate([m] * (KEYS // DH), axis=1))
        rescale = jnp.exp2(m_in - m)
        inv = 1.0 / (rescale * l_in + jnp.sum(p, axis=1, keepdims=True))
        o_in = rescale * o_in
        p = p.astype(BF16)
        v_copy(u).wait()
        ctx[h, _block(me, QBLK), :] = ((o_in + _dot(p, values(u))) * inv).astype(BF16)
        for d in send_order:
            ctx_copy(h, d, me).start()
        ready = h - PROJECT_LAG
        pl.when(ready == 0)(wo_wait)
        pl.when(jnp.logical_and(ready >= 0, ready < projected))(lambda: project_shared(ready))

    n_own = COMMON - n_foreign
    lax.fori_loop(0, n_own, own_step, None)

    k_copy(COMMON).wait()
    local_softmax(COMMON)
    for d in send_order:
        stats_copy(d).start()

    def common_half(j, o):
        p = probs[j]
        v_common_copy(j).wait()
        v = v_buf[COMMON, _block(j, KBLKS // 2)].reshape(KEYS // 2, DH)
        return o + _dot(p, v.astype(BF16))

    common[0] = lax.fori_loop(0, 2, common_half, jnp.zeros((QBLK, DH), F32)).astype(BF16)
    for d in send_order:
        common_copy(d).start()

    def wo_sent(chip):
        for t in range(len(WO_CUTS)):
            for copy in wo_outgoing(chip, t):
                copy.wait_send()

    def ctx_sent(h, _):
        for d in range(1, NDEV):
            ctx_copy(h, d, me).wait_send()

    for chip in range(NDEV):
        on(chip, lambda chip=chip: wo_sent(chip))
    for d in range(1, NDEV):
        qpart_copy(d).wait_send()
        q_copy(d, me).wait_send()
    lax.fori_loop(0, n_foreign, lambda u, _: part_copy(u).wait_send(), None)
    lax.fori_loop(0, n_own, ctx_sent, None)

    on(RELAY, lambda: wo_cast(relay_rows, w_sem.at[3]))
    lax.fori_loop(projected, SHARED_HEADS, project_shared, None)

    def common_sent():
        for d in range(1, NDEV):
            stats_copy(d).wait_send()
            common_copy(d).wait_send()

    def project_local(h, _):
        ctx_wait(h)
        pl.when(h == LAST_HEAD - 1)(common_sent)
        wo_head_copy(h).wait()
        acc[...] += _dot(ctx[h], wo_buf[_block(h, DH), :].astype(BF16))

    lax.fori_loop(SHARED_HEADS, LAST_HEAD, project_local, None)

    for d in range(1, NDEV):
        pl.when(me != d)(lambda d=d: ctx_copy(LAST_HEAD, d, peer(NDEV - d)).wait_recv())
    _wait_filled(stats.at[pl.ds(1, NDEV - 1)], stats_recv)

    owned_rows, common_rows = pl.ds(QBLK, SQ - QBLK), pl.ds(0, QBLK)
    w_last = []
    for j in range(2):
        cols = _block(j, HALF)
        wo_last_copy(j).wait()
        if j == 0:
            _, factors, total = _merge_stats([stats[d] for d in range(NDEV)])
            weights = [_spread(f / total) for f in factors]
        w_last.append(wo_buf[_block(LAST_HEAD, DH), cols].astype(BF16))
        o = acc[owned_rows, cols] + _dot(ctx[LAST_HEAD, owned_rows, :], w_last[j])
        out_ref[owned_rows, cols] = o.astype(out_ref.dtype)

    _wait_filled(common.at[pl.ds(1, NDEV - 1)], common_recv)
    t = [common[d].astype(F32) * weights[d] for d in range(NDEV)]
    merged = ((t[0] + t[2]) + (t[1] + t[3])).astype(BF16)
    o = acc[common_rows, :] + _dot(merged, jnp.concatenate(w_last, axis=1))
    out_ref[common_rows, :] = o.astype(out_ref.dtype)


def pallas_dist_sparse_attn_strided_kvseq_b1_sq256_skv4096_hq8_dh128_kernel(
    x: jax.Array,
    Wq: jax.Array,
    K_ext: jax.Array,
    V_ext: jax.Array,
    Wo: jax.Array,
):
    dma = pltpu.SemaphoreType.DMA
    peers = NDEV - 1
    kv_shape = (KBLKS, NDEV, QBLK, HEADS, DH)
    out = pl.pallas_call(
        _kernel,
        out_shape=jax.ShapeDtypeStruct((SQ, DMODEL), BF16),
        in_specs=[pl.BlockSpec(memory_space=pl.ANY)] * 5,
        out_specs=pl.BlockSpec(memory_space=pltpu.VMEM),
        scratch_shapes=[
            pltpu.VMEM((SQ, KSPLIT), F32),
            pltpu.VMEM((KSPLIT, DMODEL), F32),
            pltpu.VMEM((DMODEL, DMODEL), F32),
            pltpu.VMEM((UNITS, KBLKS, QBLK, DH), F32),
            pltpu.VMEM((UNITS, KBLKS, QBLK, DH), F32),
            pltpu.VMEM((NDEV, SQ, 2 * DH), F32),
            pltpu.VMEM((NDEV, SQ, 2 * DH), BF16),
            pltpu.VMEM((peers, SQ, 2 * DH), BF16),
            pltpu.VMEM((HEADS, SQ, DH), BF16),
            pltpu.VMEM((SHARED_HEADS * DH, DMODEL), BF16),
            pltpu.VMEM((2, QBLK, KEYS // 2), BF16),
            pltpu.VMEM((NDEV, 8, DH), F32),
            pltpu.VMEM((UNITS - HEADS, PACKED + 8, DH), U32),
            pltpu.VMEM((HEADS, peers, PACKED + 8, DH), U32),
            pltpu.VMEM((HEADS, SQ, DH), BF16),
            pltpu.VMEM((NDEV, QBLK, DH), BF16),
            pltpu.VMEM((SQ, DMODEL), F32),
            dma((4,)), dma((HEADS + 1,)), dma((UNITS,)), dma((UNITS + 1,)),
            dma((peers,)), dma, dma((peers,)), dma((peers,)),
            dma((2 * len(WO_CUTS),)), dma((NDEV * len(WO_CUTS),)),
            dma((UNITS - HEADS,)), dma((HEADS,)), dma((peers * HEADS,)), dma((peers * HEADS,)),
            dma((peers,)), dma, dma((peers,)), dma,
        ],
        compiler_params=pltpu.CompilerParams(
            collective_id=0,
            vmem_limit_bytes=64 * 1024 * 1024,
            disable_bounds_checks=True,
            disable_semaphore_checks=True,
        ),
    )(x.reshape(SQ, DMODEL), Wq, K_ext.reshape(kv_shape), V_ext.reshape(kv_shape), Wo)
    return out.reshape(1, SQ, DMODEL)
```

```python
import jax
import jax.numpy as jnp
from jax import lax
from jax.experimental import pallas as pl
from jax.experimental.pallas import tpu as pltpu

NDEV = 4
HEADS, DH = 8, 128
DMODEL = HEADS * DH
QBLK = 64
SQ = NDEV * QBLK
KBLKS = 16
KEYS = KBLKS * QBLK
UNITS = NDEV * HEADS
COMMON = UNITS - 1
LAST_HEAD = HEADS - 1
KSPLIT = DMODEL // NDEV
HALF = DMODEL // 2
PACKED = QBLK // 2

QSCALE = 0.08838834764831843 * 1.4426950408889634

WO_PIECE = {1: (0, 144), 3: (144, 192), 0: (336, 176)}
RELAY = 2
SHARED_HEADS = 4
WO_CUTS = (0, 64, 96)

PREFETCH = (9, 11, 18, 24)
LOOKAHEAD = 11
RELAY_UNIT = 5
PROJECT_LAG = 2

STAGES = ((24, 5), (25, 8), (28, 6), (29, 8), (COMMON, 4))
STAGE_UNITS = (17, 27)

F32, BF16, U32 = jnp.float32, jnp.bfloat16, jnp.uint32


def _block(index, size):
    start = index * size
    return pl.ds(start if isinstance(index, int) else pl.multiple_of(start, size), size)


def _wo_chunk(chip, t):
    first, rows = WO_PIECE[chip]
    end = WO_CUTS[t + 1] if t + 1 < len(WO_CUTS) else rows
    return pl.ds(first + WO_CUTS[t], end - WO_CUTS[t])


def _wait_filled(ref, sem):
    pltpu.make_async_copy(ref, ref, sem).wait()


def _remote(src, dst, send_sem, recv_sem, target):
    return pltpu.make_async_remote_copy(
        src, dst, send_sem, recv_sem,
        device_id=(target,), device_id_type=pl.DeviceIdType.MESH)


def _dot(a, b):
    return jnp.dot(a, b, preferred_element_type=F32)


def _pack_stats(m, l):
    lane = lax.broadcasted_iota(jnp.int32, (8, DH), 1)
    stats = jnp.zeros((8, DH), F32)
    for g in range(8):
        stats = jnp.where(lane == g, m[8 * g:8 * g + 8], stats)
        stats = jnp.where(lane == 8 + g, l[8 * g:8 * g + 8], stats)
    return stats


def _merge_stats(tiles):
    maxima = [t[:, :8] for t in tiles]
    top = maxima[0]
    for m in maxima[1:]:
        top = jnp.maximum(top, m)
    factors = [jnp.exp2(m - top) for m in maxima]
    total = sum(f * t[:, 8:16] for f, t in zip(factors, tiles))
    return top, factors, total


def _spread(packed):
    return jnp.concatenate(
        [jnp.broadcast_to(packed[:, g:g + 1], (8, DH)) for g in range(8)], axis=0)


def _kernel(
    x_hbm, wq_hbm, k_hbm, v_hbm, wo_hbm, out_ref,
    x_buf, wq_buf, wo_buf, k_buf, v_buf,
    qpart, qpart_out, qpart_in, q_all, wo_all, probs, stats,
    part_out, part_in, ctx, common, acc, stage,
    w_sem, wo_sem, k_sem, v_sem, stage_sem,
    qpart_send, qpart_recv, q_send, q_recv, wo_send, wo_recv,
    part_send, part_recv, ctx_send, ctx_recv,
    stats_send, stats_recv, common_send, common_recv,
):
    me = lax.axis_index("i")

    def peer(d):
        return (me + d) & (NDEV - 1)

    def on(chip, fn):
        pl.when(me == chip)(fn)

    n_foreign = jnp.where(me == 0, UNITS - HEADS, UNITS - HEADS - 1)

    def class_and_head(u):
        if isinstance(u, int):
            return (0, LAST_HEAD) if u == COMMON else (me, u - n_foreign)
        h = lax.div(u, NDEV - 1)
        c = NDEV - 1 - (u - (NDEV - 1) * h)
        c = jnp.where(c <= me, c - 1, c)
        foreign = u < n_foreign
        return jnp.where(foreign, c, me), jnp.where(foreign, h, u - n_foreign)

    def k_copy(u, skip=0):
        c, h = class_and_head(u)
        blocks = pl.ds(skip, KBLKS - skip)
        return pltpu.make_async_copy(k_hbm.at[blocks, c, :, h], k_buf.at[u, blocks], k_sem.at[u])

    def v_copy(u):
        c, h = class_and_head(u)
        return pltpu.make_async_copy(v_hbm.at[:, c, :, h], v_buf.at[u], v_sem.at[u])

    def stage_in(i):
        u, n = STAGES[i]
        c, h = class_and_head(u)
        return pltpu.make_async_copy(
            k_hbm.at[pl.ds(0, n), c, :, h], stage.at[i % 2, pl.ds(0, n)], stage_sem.at[0])

    def stage_out(i):
        u, n = STAGES[i]
        return pltpu.make_async_copy(
            stage.at[i % 2, pl.ds(0, n)], k_buf.at[u, pl.ds(0, n)], stage_sem.at[1])

    def stage_step(p):
        if p >= 2:
            stage_out(p - 2).wait()
        if 1 <= p <= len(STAGES):
            stage_in(p - 1).wait()
            stage_out(p - 1).start()
        if p < len(STAGES):
            stage_in(p).start()

    staged = dict(STAGES)

    def with_direct_k(u, action):
        for unit in range(UNITS - HEADS - 1, COMMON):
            pl.when(u == unit)(lambda unit=unit: action(k_copy(unit, staged.get(unit, 0))))

    def v_common_copy(j):
        blocks = _block(j, KBLKS // 2)
        return pltpu.make_async_copy(
            v_hbm.at[blocks, 0, :, LAST_HEAD], v_buf.at[COMMON, blocks], v_sem.at[COMMON + j])

    def wo_copy(rows, sem, cols=pl.ds(0, DMODEL)):
        return pltpu.make_async_copy(wo_hbm.at[rows, cols], wo_buf.at[rows, cols], sem)

    def wo_head_copy(h):
        return wo_copy(_block(h, DH), wo_sem.at[h])

    def wo_last_copy(j):
        return wo_copy(_block(LAST_HEAD, DH), wo_sem.at[LAST_HEAD + j], _block(j, HALF))

    def wo_cast(rows, sem):
        wo_copy(rows, sem).wait()
        wo_all[rows, :] = wo_buf[rows, :].astype(BF16)

    def wo_rest(chip):
        first, rows = WO_PIECE[chip]
        return pl.ds(first + WO_CUTS[1], rows - WO_CUTS[1])

    def fetch(u, _):
        k_copy(u).start()
        v_copy(u).start()

    def qpart_copy(d):
        return _remote(qpart_out.at[peer(d)], qpart_in.at[d - 1],
                       qpart_send.at[d - 1], qpart_recv, peer(d))

    def q_copy(d, owner):
        heads = q_all.at[pl.ds(2 * owner, 2)]
        return _remote(heads, heads, q_send.at[d - 1], q_recv.at[d - 1], peer(d))

    def wo_share_copy(chip, t, side, target):
        rows = wo_all.at[_wo_chunk(chip, t)]
        return _remote(rows, rows, wo_send.at[2 * t + side], wo_recv.at[NDEV * t + chip], target)

    def wo_outgoing(sender, t):
        if sender == RELAY:
            return [wo_share_copy(1, t, 0, 3), wo_share_copy(3, t, 1, 1)]
        return [wo_share_copy(sender, t, side, (sender + d) % NDEV)
                for side, d in enumerate((1, 3))]

    def wo_forward(sender, t):
        if sender == RELAY:
            for copy in wo_outgoing(sender, t):
                copy.wait_recv()
        for copy in wo_outgoing(sender, t):
            copy.start()

    def part_copy(u):
        c, h = class_and_head(u)
        return _remote(part_out.at[u], part_in.at[h, jnp.where(me > c, me - 1, me)],
                       part_send.at[u], part_recv.at[h], c)

    def ctx_copy(h, d, owner):
        rows = ctx.at[h, _block(owner, QBLK)]
        slot = (NDEV - 1) * h + d - 1
        return _remote(rows, rows, ctx_send.at[slot], ctx_recv.at[slot], peer(d))

    def stats_copy(d):
        return _remote(stats.at[0], stats.at[d], stats_send.at[d - 1], stats_recv, peer(d))

    def common_copy(d):
        return _remote(common.at[0], common.at[d], common_send.at[d - 1], common_recv, peer(d))

    def load_projection(j, _):
        rows = _block(j, SQ // 2)
        pltpu.make_async_copy(
            x_hbm.at[rows, _block(me, KSPLIT)], x_buf.at[rows], w_sem.at[0]).start()
        pltpu.make_async_copy(
            wq_hbm.at[_block(2 * me + j, KSPLIT // 2)], wq_buf.at[_block(j, KSPLIT // 2)],
            w_sem.at[1]).start()

    for chip in WO_PIECE:
        on(chip, lambda chip=chip: wo_copy(_wo_chunk(chip, 0), w_sem.at[2]).start())
    lax.fori_loop(0, 2, load_projection, None)
    for chip in WO_PIECE:
        on(chip, lambda chip=chip: wo_copy(wo_rest(chip), w_sem.at[3]).start())

    stage_step(0)

    barrier = pltpu.get_barrier_semaphore()
    for d in (2, 1, 3):
        pl.semaphore_signal(barrier, inc=1, device_id=(peer(d),),
                            device_id_type=pl.DeviceIdType.MESH)
    lax.fori_loop(0, PREFETCH[0], fetch, None)
    acc[...] = jnp.zeros(acc.shape, F32)

    for chip in WO_PIECE:
        on(chip, lambda chip=chip: wo_cast(_wo_chunk(chip, 0), w_sem.at[2]))
    pl.semaphore_wait(barrier, NDEV - 1)
    for chip in WO_PIECE:
        on(chip, lambda chip=chip: wo_forward(chip, 0))

    _wait_filled(x_buf, w_sem.at[0])
    _wait_filled(wq_buf, w_sem.at[1])
    q = _dot(x_buf[...].astype(BF16), wq_buf[...].astype(BF16)) * QSCALE
    for j in range(NDEV):
        q_cols = q[:, 2 * DH * j:2 * DH * (j + 1)]
        qpart[j] = q_cols
        qpart_out[j] = q_cols.astype(BF16)
    for d in (1, 3, 2):
        qpart_copy(d).start()

    for chip in WO_PIECE:
        on(chip, lambda chip=chip: wo_cast(wo_rest(chip), w_sem.at[3]))
    for chip in WO_PIECE:
        on(chip, lambda chip=chip: wo_forward(chip, 1))
    lax.fori_loop(PREFETCH[0], PREFETCH[1], fetch, None)
    stage_step(1)
    on(RELAY, lambda: wo_forward(RELAY, 0))

    _wait_filled(qpart_in, qpart_recv)
    lax.fori_loop(PREFETCH[1], PREFETCH[2], fetch, None)
    q = qpart[me] + sum(qpart_in[j].astype(F32) for j in range(NDEV - 1))
    q_all[2 * me] = q[:, :DH].astype(BF16)
    q_all[2 * me + 1] = q[:, DH:].astype(BF16)
    for d in (1, 3, 2):
        q_copy(d, me).start()

    for chip in WO_PIECE:
        on(chip, lambda chip=chip: wo_forward(chip, 2))
    stage_step(2)
    on(RELAY, lambda: wo_forward(RELAY, 1))

    for d in (1, 3, 2):
        q_copy(d, peer(NDEV - d)).wait_recv()
    lax.fori_loop(PREFETCH[2], PREFETCH[3], fetch, None)
    stage_step(3)

    def scores(u):
        c, h = class_and_head(u)
        k = k_buf[u].reshape(KEYS, DH).astype(BF16)
        return lax.dot_general(q_all[h, _block(c, QBLK), :], k, (((1,), (1,)), ((), ())),
                               preferred_element_type=F32)

    def values(u):
        return v_buf[u].reshape(KEYS, DH).astype(BF16)

    def local_softmax(u):
        s = scores(u)
        m = jnp.max(s, axis=1, keepdims=True)
        p = jnp.exp2(s - m)
        stats[0] = _pack_stats(m, jnp.sum(p, axis=1, keepdims=True))
        probs[0] = p[:, :KEYS // 2].astype(BF16)
        probs[1] = p[:, KEYS // 2:].astype(BF16)

    def store_partial(u):
        o = _dot(jnp.concatenate([probs[0], probs[1]], axis=1), values(u))
        part_out[u, pl.ds(PACKED, 8), :] = pltpu.bitcast(stats[0], U32)
        part_out[u, pl.ds(0, PACKED), :] = pltpu.bitcast(o.astype(BF16), U32)

    def foreign_step(u, _):
        ahead = u + LOOKAHEAD
        refill = jnp.logical_and(ahead >= PREFETCH[3], ahead < COMMON)
        pl.when(refill)(lambda: with_direct_k(ahead, lambda copy: copy.start()))
        pl.when(u == STAGE_UNITS[0])(lambda: stage_step(4))
        pl.when(jnp.logical_and(u == RELAY_UNIT, me == RELAY))(lambda: wo_forward(RELAY, 2))
        v_copy(u).wait()
        k_copy(u + 1).wait()
        pl.when(refill)(lambda: v_copy(ahead).start())
        store_partial(u)
        local_softmax(u + 1)
        part_copy(u).start()

    k_copy(jnp.int32(0)).wait()
    local_softmax(jnp.int32(0))
    lax.fori_loop(0, n_foreign - 1, foreign_step, None)
    v_copy(n_foreign - 1).wait()
    store_partial(n_foreign - 1)
    part_copy(n_foreign - 1).start()

    first = jnp.where(me == 0, 1, NDEV - me)
    second = jnp.where(first == 2, 1, NDEV - first)
    send_order = (first, second, 6 - first - second)

    def ctx_wait(h):
        for d in range(1, NDEV):
            ctx_copy(h, d, peer(NDEV - d)).wait_recv()

    def project_shared(h, _=None):
        ctx_wait(h)
        acc[...] += _dot(ctx[h], wo_all[_block(h, DH), :])

    def wo_arrivals(chip):
        for t in range(len(WO_CUTS)):
            for source in WO_PIECE:
                if source != chip:
                    wo_share_copy(source, t, 0, source).wait_recv()

    def wo_wait():
        for chip in WO_PIECE:
            on(chip, lambda chip=chip: wo_arrivals(chip))

    relay_rows = pl.ds(*WO_PIECE[0])
    late_reads = (
        lambda: k_copy(COMMON, staged[COMMON]).start(),
        lambda: v_common_copy(0).start(),
        lambda: v_common_copy(1).start(),
        lambda: on(RELAY, lambda: wo_copy(relay_rows, w_sem.at[3]).start()),
        lambda: lax.fori_loop(SHARED_HEADS, LAST_HEAD, lambda h, _: wo_head_copy(h).start(), None),
        lambda: wo_last_copy(0).start(),
        lambda: wo_last_copy(1).start(),
    )
    projected = jnp.where(me == RELAY, WO_PIECE[0][0] // DH, SHARED_HEADS - 1)

    def own_step(h, _):
        for step, start in enumerate(late_reads):
            pl.when(h == step)(start)
        u = n_foreign + h
        _wait_filled(part_in.at[h], part_recv.at[h])
        m_in, factors, l_in = _merge_stats(
            [pltpu.bitcast(part_in[h, j, pl.ds(PACKED, 8), :], F32) for j in range(NDEV - 1)])
        m_in, l_in = _spread(m_in), _spread(l_in)
        o_in = sum(
            _spread(f) * pltpu.bitcast(part_in[h, j, pl.ds(0, PACKED), :], BF16).astype(F32)
            for j, f in enumerate(factors))
        with_direct_k(u, lambda copy: copy.wait())
        s = scores(u)
        m = jnp.maximum(m_in, jnp.max(s, axis=1, keepdims=True))
        p = jnp.exp2(s - jnp.concatenate([m] * (KEYS // DH), axis=1))
        rescale = jnp.exp2(m_in - m)
        inv = 1.0 / (rescale * l_in + jnp.sum(p, axis=1, keepdims=True))
        o_in = rescale * o_in
        p = p.astype(BF16)
        pl.when(u == STAGE_UNITS[1])(lambda: stage_step(5))
        v_copy(u).wait()
        ctx[h, _block(me, QBLK), :] = ((o_in + _dot(p, values(u))) * inv).astype(BF16)
        for d in send_order:
            ctx_copy(h, d, me).start()
        ready = h - PROJECT_LAG
        pl.when(ready == 0)(wo_wait)
        pl.when(jnp.logical_and(ready >= 0, ready < projected))(lambda: project_shared(ready))

    n_own = COMMON - n_foreign
    lax.fori_loop(0, n_own, own_step, None)

    stage_step(6)
    k_copy(COMMON, staged[COMMON]).wait()
    local_softmax(COMMON)
    for d in send_order:
        stats_copy(d).start()

    def common_half(j, o):
        p = probs[j]
        v_common_copy(j).wait()
        v = v_buf[COMMON, _block(j, KBLKS // 2)].reshape(KEYS // 2, DH)
        return o + _dot(p, v.astype(BF16))

    common[0] = lax.fori_loop(0, 2, common_half, jnp.zeros((QBLK, DH), F32)).astype(BF16)
    for d in send_order:
        common_copy(d).start()

    def wo_sent(chip):
        for t in range(len(WO_CUTS)):
            for copy in wo_outgoing(chip, t):
                copy.wait_send()

    def ctx_sent(h, _):
        for d in range(1, NDEV):
            ctx_copy(h, d, me).wait_send()

    for chip in range(NDEV):
        on(chip, lambda chip=chip: wo_sent(chip))
    for d in range(1, NDEV):
        qpart_copy(d).wait_send()
        q_copy(d, me).wait_send()
    lax.fori_loop(0, n_foreign, lambda u, _: part_copy(u).wait_send(), None)
    lax.fori_loop(0, n_own, ctx_sent, None)

    on(RELAY, lambda: wo_cast(relay_rows, w_sem.at[3]))
    lax.fori_loop(projected, SHARED_HEADS, project_shared, None)

    def common_sent():
        for d in range(1, NDEV):
            stats_copy(d).wait_send()
            common_copy(d).wait_send()

    def project_local(h, _):
        ctx_wait(h)
        pl.when(h == LAST_HEAD - 1)(common_sent)
        wo_head_copy(h).wait()
        acc[...] += _dot(ctx[h], wo_buf[_block(h, DH), :].astype(BF16))

    lax.fori_loop(SHARED_HEADS, LAST_HEAD, project_local, None)

    for d in range(1, NDEV):
        pl.when(me != d)(lambda d=d: ctx_copy(LAST_HEAD, d, peer(NDEV - d)).wait_recv())
    _wait_filled(stats.at[pl.ds(1, NDEV - 1)], stats_recv)

    owned_rows, common_rows = pl.ds(QBLK, SQ - QBLK), pl.ds(0, QBLK)
    w_last = []
    for j in range(2):
        cols = _block(j, HALF)
        wo_last_copy(j).wait()
        if j == 0:
            _, factors, total = _merge_stats([stats[d] for d in range(NDEV)])
            weights = [_spread(f / total) for f in factors]
        w_last.append(wo_buf[_block(LAST_HEAD, DH), cols].astype(BF16))
        o = acc[owned_rows, cols] + _dot(ctx[LAST_HEAD, owned_rows, :], w_last[j])
        out_ref[owned_rows, cols] = o.astype(out_ref.dtype)

    _wait_filled(common.at[pl.ds(1, NDEV - 1)], common_recv)
    t = [common[d].astype(F32) * weights[d] for d in range(NDEV)]
    merged = ((t[0] + t[2]) + (t[1] + t[3])).astype(BF16)
    o = acc[common_rows, :] + _dot(merged, jnp.concatenate(w_last, axis=1))
    out_ref[common_rows, :] = o.astype(out_ref.dtype)


def pallas_dist_sparse_attn_strided_kvseq_b1_sq256_skv4096_hq8_dh128_kernel(
    x: jax.Array,
    Wq: jax.Array,
    K_ext: jax.Array,
    V_ext: jax.Array,
    Wo: jax.Array,
):
    dma = pltpu.SemaphoreType.DMA
    peers = NDEV - 1
    kv_shape = (KBLKS, NDEV, QBLK, HEADS, DH)
    out = pl.pallas_call(
        _kernel,
        out_shape=jax.ShapeDtypeStruct((SQ, DMODEL), BF16),
        in_specs=[pl.BlockSpec(memory_space=pl.ANY)] * 5,
        out_specs=pl.BlockSpec(memory_space=pltpu.VMEM),
        scratch_shapes=[
            pltpu.VMEM((SQ, KSPLIT), F32),
            pltpu.VMEM((KSPLIT, DMODEL), F32),
            pltpu.VMEM((DMODEL, DMODEL), F32),
            pltpu.VMEM((UNITS, KBLKS, QBLK, DH), F32),
            pltpu.VMEM((UNITS, KBLKS, QBLK, DH), F32),
            pltpu.VMEM((NDEV, SQ, 2 * DH), F32),
            pltpu.VMEM((NDEV, SQ, 2 * DH), BF16),
            pltpu.VMEM((peers, SQ, 2 * DH), BF16),
            pltpu.VMEM((HEADS, SQ, DH), BF16),
            pltpu.VMEM((SHARED_HEADS * DH, DMODEL), BF16),
            pltpu.VMEM((2, QBLK, KEYS // 2), BF16),
            pltpu.VMEM((NDEV, 8, DH), F32),
            pltpu.VMEM((UNITS - HEADS, PACKED + 8, DH), U32),
            pltpu.VMEM((HEADS, peers, PACKED + 8, DH), U32),
            pltpu.VMEM((HEADS, SQ, DH), BF16),
            pltpu.VMEM((NDEV, QBLK, DH), BF16),
            pltpu.VMEM((SQ, DMODEL), F32),
            pltpu.SMEM((2, max(n for _, n in STAGES), QBLK, DH), F32),
            dma((4,)), dma((HEADS + 1,)), dma((UNITS,)), dma((UNITS + 1,)),
            dma((2,)),
            dma((peers,)), dma, dma((peers,)), dma((peers,)),
            dma((2 * len(WO_CUTS),)), dma((NDEV * len(WO_CUTS),)),
            dma((UNITS - HEADS,)), dma((HEADS,)), dma((peers * HEADS,)), dma((peers * HEADS,)),
            dma((peers,)), dma, dma((peers,)), dma,
        ],
        compiler_params=pltpu.CompilerParams(
            collective_id=0,
            vmem_limit_bytes=64 * 1024 * 1024,
            disable_bounds_checks=True,
            disable_semaphore_checks=True,
        ),
    )(x.reshape(SQ, DMODEL), Wq, K_ext.reshape(kv_shape), V_ext.reshape(kv_shape), Wo)
    return out.reshape(1, SQ, DMODEL)
```
